```python
import numpy as np

kernel_name = "dist_mean_ax0_shard0_i_m2048_n1024"

def setup_inputs():
    return {"x": np.random.randn(8192, 1024).astype(np.float32)}

def reference(x: np.ndarray) -> np.ndarray:
    return np.mean(x, axis=0, keepdims=True)
```

```python
import jax
import jax.numpy as jnp
from jax import lax
from jax.experimental import pallas as pl
from jax.experimental.pallas import tpu as pltpu

N_DEV = 4
SUBLANES = 8
CHUNKS = (256, 256, 256, 256, 256, 256, 256, 256)


def pallas_dist_mean_ax0_shard0_i_m2048_n1024_kernel(
x: jax.Array,
):
    m, n = x.shape
    assert sum(CHUNKS) == m
    starts = [sum(CHUNKS[:c]) for c in range(len(CHUNKS))]
    scale = 1.0 / (m * N_DEV)

    def kernel_body(x_hbm, out_ref, buf, parts, load_sems, send_sems, recv_sems):
        loads = [
            pltpu.make_async_copy(
                x_hbm.at[pl.ds(s, r)], buf.at[pl.ds(s, r)], load_sems.at[c]
            )
            for c, (s, r) in enumerate(zip(starts, CHUNKS))
        ]
        for load in loads:
            load.start()

        me = lax.axis_index("i")
        peers = [(me + k) % N_DEV for k in range(1, N_DEV)]
        barrier = pltpu.get_barrier_semaphore()
        for peer in peers:
            pl.semaphore_signal(
                barrier, inc=1, device_id=(peer,),
                device_id_type=pl.DeviceIdType.MESH,
            )

        acc = jnp.zeros((SUBLANES, n), jnp.float32)
        for load, s, r in zip(loads, starts, CHUNKS):
            load.wait()
            acc = acc + jnp.sum(
                buf[pl.ds(s, r), :].reshape(r // SUBLANES, SUBLANES, n), axis=0
            )
        parts[0] = jnp.sum(acc, axis=0, keepdims=True)

        pl.semaphore_wait(barrier, N_DEV - 1)
        sends = [
            pltpu.make_async_remote_copy(
                src_ref=parts.at[0],
                dst_ref=parts.at[k],
                send_sem=send_sems.at[k - 1],
                recv_sem=recv_sems.at[k - 1],
                device_id=(peer,),
                device_id_type=pl.DeviceIdType.MESH,
            )
            for k, peer in enumerate(peers, start=1)
        ]
        for send in sends:
            send.start()
        for send in sends:
            send.wait_recv()
        out_ref[...] = ((parts[0] + parts[1]) + (parts[2] + parts[3])) * scale
        for send in sends:
            send.wait_send()

    return pl.pallas_call(
        kernel_body,
        out_shape=jax.ShapeDtypeStruct((1, n), x.dtype),
        in_specs=[pl.BlockSpec(memory_space=pl.ANY)],
        out_specs=pl.BlockSpec(memory_space=pltpu.VMEM),
        scratch_shapes=[
            pltpu.VMEM((m, n), x.dtype),
            pltpu.VMEM((N_DEV, 1, n), jnp.float32),
            pltpu.SemaphoreType.DMA((len(CHUNKS),)),
            pltpu.SemaphoreType.DMA((N_DEV - 1,)),
            pltpu.SemaphoreType.DMA((N_DEV - 1,)),
        ],
        compiler_params=pltpu.CompilerParams(collective_id=0),
    )(x)
```

```python
import jax
import jax.numpy as jnp
from jax import lax
from jax.experimental import pallas as pl
from jax.experimental.pallas import tpu as pltpu

N_DEV = 4
ROWS = 8
WAYS = 8
AHEAD = 16
TAIL = (6, 1, 1)


def pallas_dist_mean_ax0_shard0_i_m2048_n1024_kernel(
x: jax.Array,
):
    m, n = x.shape
    step_rows = WAYS * ROWS
    steps = m // step_rows
    way_stride = m // WAYS
    scale = 1.0 / (m * N_DEV)
    tail_of = [g for g, c in enumerate(TAIL) for _ in range(c)]

    def kernel_body(x_hbm, out_ref, buf, parts, load_sems, send_sems, recv_sems):
        def issue(s, last=False):
            for w in range(WAYS):
                src = w * way_stride + s * ROWS
                dst = s * step_rows + w * ROWS
                if not isinstance(s, int):
                    src, dst = pl.multiple_of(src, ROWS), pl.multiple_of(dst, ROWS)
                pltpu.make_async_copy(
                    x_hbm.at[pl.ds(src, ROWS)],
                    buf.at[pl.ds(dst, ROWS)],
                    load_sems.at[s + tail_of[w] if last else s],
                ).start(priority=w % 2)

        def consume(start, rows, sem):
            if not isinstance(start, int):
                start = pl.multiple_of(start, ROWS)
            blk = buf.at[pl.ds(start, rows)]
            pltpu.make_async_copy(blk, blk, sem).wait()
            return jnp.sum(blk[...].reshape(rows // ROWS, ROWS, n), axis=0)

        for s in range(AHEAD):
            issue(s)

        me = lax.axis_index("i")
        peer = {k: lax.rem(me + k, N_DEV) for k in range(1, N_DEV)}
        barrier = pltpu.get_barrier_semaphore()
        for k in peer:
            pl.semaphore_signal(
                barrier, inc=1, device_id=(peer[k],),
                device_id_type=pl.DeviceIdType.MESH,
            )

        def main(s, acc):
            issue(s + AHEAD)
            return acc + consume(s * step_rows, step_rows, load_sems.at[s])

        def drain(s, acc):
            return acc + consume(s * step_rows, step_rows, load_sems.at[s])

        acc = jnp.zeros((ROWS, n), jnp.float32)
        acc = lax.fori_loop(0, steps - AHEAD - 1, main, acc)
        issue(steps - 1, last=True)
        acc = lax.fori_loop(steps - AHEAD - 1, steps - 1, drain, acc)
        pl.semaphore_wait(barrier, N_DEV - 1)
        off = (steps - 1) * step_rows
        for g, c in enumerate(TAIL):
            acc = acc + consume(off, c * ROWS, load_sems.at[steps - 1 + g])
            off += c * ROWS
        parts[0] = jnp.sum(acc, axis=0, keepdims=True)

        sends = {
            k: pltpu.make_async_remote_copy(
                src_ref=parts.at[0],
                dst_ref=parts.at[k],
                send_sem=send_sems.at[k - 1],
                recv_sem=recv_sems.at[k - 1],
                device_id=(peer[k],),
                device_id_type=pl.DeviceIdType.MESH,
            )
            for k in peer
        }
        for k in (2, 1, 3):
            sends[k].start()
        for k in peer:
            sends[k].wait_send()
        sends[1].wait_recv()
        sends[3].wait_recv()
        near = (parts[0] + parts[1]) + parts[3]
        sends[2].wait_recv()
        out_ref[...] = (near + parts[2]) * scale

    return pl.pallas_call(
        kernel_body,
        out_shape=jax.ShapeDtypeStruct((1, n), x.dtype),
        in_specs=[pl.BlockSpec(memory_space=pl.ANY)],
        out_specs=pl.BlockSpec(memory_space=pltpu.VMEM),
        scratch_shapes=[
            pltpu.VMEM((m, n), x.dtype),
            pltpu.VMEM((N_DEV, 1, n), jnp.float32),
            pltpu.SemaphoreType.DMA((steps + len(TAIL) - 1,)),
            pltpu.SemaphoreType.DMA((N_DEV - 1,)),
            pltpu.SemaphoreType.DMA((N_DEV - 1,)),
        ],
        compiler_params=pltpu.CompilerParams(
            collective_id=0,
            disable_bounds_checks=True,
            disable_semaphore_checks=True,
        ),
    )(x)
```

```python
import jax
import jax.numpy as jnp
from jax import lax
from jax.experimental import pallas as pl
from jax.experimental.pallas import tpu as pltpu

N_DEV = 4
ROWS = 8
WAYS = 8
LEAD = 7
AHEAD = 8
LATE_STEPS = 3
LATE_COLS = 128
LATE_GROUPS = (20, 3, 1)


def pallas_dist_mean_ax0_shard0_i_m2048_n1024_kernel(
x: jax.Array,
):
    m, n = x.shape
    step_rows = WAYS * ROWS
    steps = m // step_rows
    full_steps = steps - LATE_STEPS
    loop_steps = full_steps - LEAD - AHEAD
    early_cols = n - LATE_COLS
    late_group = [g for g, size in enumerate(LATE_GROUPS) for _ in range(size)]
    first_late_turn = (steps + LEAD) * (WAYS // 2) - len(late_group)
    assert m % step_rows == 0 and loop_steps >= 0
    assert len(late_group) == LATE_STEPS * WAYS <= LEAD * (WAYS // 2)

    def kernel_body(
        x_hbm, out_ref, full, early, late, sums,
        step_sems, late_sems, send_sems, recv_sems,
    ):
        def rows(start, size):
            if not isinstance(start, int):
                start = pl.multiple_of(start, ROWS)
            return pl.ds(start, size)

        def shard_rows(step, way):
            return rows(way * (m // WAYS) + step * ROWS, ROWS)

        def fetch_piece(step, way, priority):
            if isinstance(step, int) and step >= full_steps:
                src = x_hbm.at[shard_rows(step, way), pl.ds(0, early_cols)]
                dst = early.at[rows((step - full_steps) * step_rows + way * ROWS, ROWS)]
            else:
                src = x_hbm.at[shard_rows(step, way)]
                dst = full.at[rows(step * step_rows + way * ROWS, ROWS)]
            pltpu.make_async_copy(src, dst, step_sems.at[step]).start(priority=priority)

        def fetch_late_tile(tile):
            step, way = full_steps + tile // WAYS, tile % WAYS
            pltpu.make_async_copy(
                x_hbm.at[shard_rows(step, way), pl.ds(early_cols, LATE_COLS)],
                late.at[rows(tile * ROWS, ROWS)],
                late_sems.at[late_group[tile]],
            ).start(priority=1)

        def prime(step):
            for j in range(WAYS // 2):
                fetch_piece(step, 2 * j, 1)

        def fetch(step):
            for j in range(WAYS // 2):
                fetch_piece(step, 2 * j + 1, 0)
                if not isinstance(step, int) or step + LEAD < steps:
                    fetch_piece(step + LEAD, 2 * j, 1)
                else:
                    tile = (step + LEAD) * (WAYS // 2) + j - first_late_turn
                    if tile >= 0:
                        fetch_late_tile(tile)

        def landed_sum(block, sem):
            pltpu.make_async_copy(block, block, sem).wait()
            size, cols = block.shape
            return jnp.sum(block[...].reshape(size // ROWS, ROWS, cols), axis=0)

        def add_full_step(step, acc):
            block = full.at[rows(step * step_rows, step_rows)]
            return acc + landed_sum(block, step_sems.at[step])

        def fetch_and_add(step, acc):
            fetch(step + AHEAD)
            return add_full_step(step, acc)

        pl.loop(0, LEAD)(prime)
        pl.loop(0, AHEAD)(fetch)

        me = lax.axis_index("i")
        peers = [lax.rem(me + hop, N_DEV) for hop in range(N_DEV)]
        barrier = pltpu.get_barrier_semaphore()
        for peer in peers[1:]:
            pl.semaphore_signal(
                barrier, inc=1, device_id=(peer,),
                device_id_type=pl.DeviceIdType.MESH,
            )

        acc = jnp.zeros((ROWS, n), jnp.float32)
        acc = lax.fori_loop(0, loop_steps, fetch_and_add, acc)
        for step in range(loop_steps + AHEAD, steps):
            fetch(step)
        acc = lax.fori_loop(loop_steps, full_steps, add_full_step, acc)

        pl.semaphore_wait(barrier, N_DEV - 1)

        def message(slot, hop, start, size):
            return pltpu.make_async_remote_copy(
                src_ref=sums.at[0, :, pl.ds(start, size)],
                dst_ref=sums.at[hop, :, pl.ds(start, size)],
                send_sem=send_sems.at[slot],
                recv_sem=recv_sems.at[slot],
                device_id=(peers[hop],),
                device_id_type=pl.DeviceIdType.MESH,
            )

        far = [message(0, 2, 0, early_cols), message(1, 2, early_cols, LATE_COLS)]
        near = [message(2, 1, 0, n), message(3, 3, 0, n)]

        acc_early, acc_late = acc[:, :early_cols], acc[:, early_cols:]
        for step in range(full_steps, steps):
            block = early.at[rows((step - full_steps) * step_rows, step_rows)]
            acc_early = acc_early + landed_sum(block, step_sems.at[step])
        sums[0, :, pl.ds(0, early_cols)] = jnp.sum(acc_early, axis=0, keepdims=True)
        far[0].start()

        for group, size in enumerate(LATE_GROUPS):
            block = late.at[rows(sum(LATE_GROUPS[:group]) * ROWS, size * ROWS)]
            acc_late = acc_late + landed_sum(block, late_sems.at[group])
        sums[0, :, pl.ds(early_cols, LATE_COLS)] = jnp.sum(
            acc_late, axis=0, keepdims=True
        )
        far[1].start()
        for copy in near:
            copy.start()

        for copy in far + near:
            copy.wait_send()
        for copy in near:
            copy.wait_recv()
        neighbours = sums[1] + sums[3]
        for copy in far:
            copy.wait_recv()
        total = (sums[0] + sums[2]) + neighbours
        out_ref[...] = (total * (1.0 / (m * N_DEV))).astype(out_ref.dtype)

    return pl.pallas_call(
        kernel_body,
        out_shape=jax.ShapeDtypeStruct((1, n), x.dtype),
        in_specs=[pl.BlockSpec(memory_space=pl.ANY)],
        out_specs=pl.BlockSpec(memory_space=pltpu.VMEM),
        scratch_shapes=[
            pltpu.VMEM((full_steps * step_rows, n), x.dtype),
            pltpu.VMEM((LATE_STEPS * step_rows, early_cols), x.dtype),
            pltpu.VMEM((LATE_STEPS * step_rows, LATE_COLS), x.dtype),
            pltpu.VMEM((N_DEV, 1, n), jnp.float32),
            pltpu.SemaphoreType.DMA((steps,)),
            pltpu.SemaphoreType.DMA((len(LATE_GROUPS),)),
            pltpu.SemaphoreType.DMA((4,)),
            pltpu.SemaphoreType.DMA((4,)),
        ],
        compiler_params=pltpu.CompilerParams(
            collective_id=0,
            disable_semaphore_checks=True,
        ),
    )(x)
```
